```python
import numpy as np

kernel_name = "dist_sum_ax1_xy_m512_n256"

def setup_inputs():
    return {"x": np.random.randn(1024, 512).astype(np.float32)}

def reference(x: np.ndarray) -> np.ndarray:
    return np.sum(x, axis=1, keepdims=True)
```

```python
import jax
import jax.numpy as jnp
from jax import lax
from jax.experimental import pallas as pl
from jax.experimental.pallas import tpu as pltpu

LANES = 128
SUB = 8


RAW = 32
H = (80, 80, 56, 32)


def pallas_dist_sum_ax1_xy_m512_n256_kernel(x):
    m, n = x.shape
    assert (m, n) == (512, 256)
    raw_lo = m - RAW
    chunks = ((0, 256), (256, 128), (384, raw_lo - 384))

    def body(x_hbm, out_ref, xbuf, send_buf, recv_buf, peer_rows, load_sems, send_sems, recv_sems):
        def load(i, lo, rows):
            return pltpu.make_async_copy(x_hbm.at[pl.ds(lo, rows)], xbuf.at[pl.ds(lo, rows)], load_sems.at[i])

        loads = [load(i, lo, rows) for i, (lo, rows) in enumerate(chunks)]
        for cp in loads:
            cp.start()

        peer = (lax.axis_index("x"), 1 - lax.axis_index("y"))
        barrier = pltpu.get_barrier_semaphore()
        pl.semaphore_signal(barrier, inc=1, device_id=peer, device_id_type=pl.DeviceIdType.MESH)
        pl.semaphore_wait(barrier, 1)

        def remote(i, src, dst):
            return pltpu.make_async_remote_copy(
                src_ref=src, dst_ref=dst, send_sem=send_sems.at[i], recv_sem=recv_sems.at[i],
                device_id=peer, device_id_type=pl.DeviceIdType.MESH)

        raw = remote(3, x_hbm.at[pl.ds(raw_lo, RAW)], peer_rows)
        raw.start()

        sub = lax.broadcasted_iota(jnp.int32, (SUB, LANES), 0)
        lane = lax.broadcasted_iota(jnp.int32, (SUB, LANES), 1)
        diag = (lane & (SUB - 1)) == sub
        group = lane >> 3

        def fold(ref, lo, hi):
            return ref[lo:hi, 0:LANES] + ref[lo:hi, LANES:2 * LANES]

        def lane_sums(vals, g0, keep):
            acc = None
            for i, v in enumerate(vals):
                s = jnp.broadcast_to(jnp.sum(v, axis=1, keepdims=True), (SUB, LANES))
                acc = s if acc is None else jnp.where(group == g0 + i, s, acc)
            return jnp.sum(jnp.where(keep, acc, 0.0), axis=0, keepdims=True)

        def tile_sums(t, rows):
            base, h = LANES * t, H[t]
            keep = diag if rows == LANES else jnp.logical_and(diag, lane < rows)
            vals = [fold(xbuf, base + r, base + r + SUB) for r in range(h, rows, SUB)]
            send_buf[:, base:base + LANES] = lane_sums(vals, h // SUB, keep)
            if h:
                send_buf[:, base:base + h] = lax.dot_general(
                    jnp.ones((SUB, LANES), jnp.float32), fold(xbuf, base, base + h),
                    (((1,), (1,)), ((), ())), preferred_element_type=jnp.float32)[0:1]

        def send(i, lo, hi):
            cp = remote(i, send_buf.at[:, pl.ds(lo, hi - lo)], recv_buf.at[:, pl.ds(lo, hi - lo)])
            cp.start()
            return cp

        loads[0].wait()
        tile_sums(0, LANES)
        tile_sums(1, LANES)
        s0 = send(0, 0, 256)
        loads[1].wait()
        tile_sums(2, LANES)
        s1 = send(1, 256, 384)
        loads[2].wait()
        tile_sums(3, raw_lo - 384)
        s2 = send(2, 384, 512)

        own_raw = load(3, raw_lo, RAW)
        own_raw.start()
        s0.wait_send()
        s1.wait_send()
        s2.wait_send()
        raw.wait_send()
        own_raw.wait()
        raw.wait_recv()
        vals = [fold(xbuf, raw_lo + r, raw_lo + r + SUB) + fold(peer_rows, r, r + SUB) for r in range(0, RAW, SUB)]
        g0 = (raw_lo - 384) // SUB
        own3 = send_buf[:, 384:512] + lane_sums(vals, g0, jnp.logical_and(diag, lane >= raw_lo - 384))
        s0.wait_recv()
        out_ref[:, 0:256] = send_buf[:, 0:256] + recv_buf[:, 0:256]
        s1.wait_recv()
        out_ref[:, 256:384] = send_buf[:, 256:384] + recv_buf[:, 256:384]
        s2.wait_recv()
        out_ref[:, 384:512] = own3 + recv_buf[:, 384:512]

    out = pl.pallas_call(
        body,
        out_shape=jax.ShapeDtypeStruct((1, m), x.dtype),
        in_specs=[pl.BlockSpec(memory_space=pl.ANY)],
        out_specs=pl.BlockSpec(memory_space=pltpu.VMEM),
        scratch_shapes=[
            pltpu.VMEM((m, n), jnp.float32),
            pltpu.VMEM((1, m), jnp.float32),
            pltpu.VMEM((1, m), jnp.float32),
            pltpu.VMEM((RAW, n), jnp.float32),
            pltpu.SemaphoreType.DMA((4,)),
            pltpu.SemaphoreType.DMA((4,)),
            pltpu.SemaphoreType.DMA((4,)),
        ],
        compiler_params=pltpu.CompilerParams(collective_id=0, disable_semaphore_checks=True),
    )(x)
    return out.reshape(m, 1)
```

```python
import jax
import jax.numpy as jnp
from jax import lax
from jax.experimental import pallas as pl
from jax.experimental.pallas import tpu as pltpu

LANES = 128
SUB = 8
RAW = 32
MXU_ROWS = (80, 80, 56, 32)


def pallas_dist_sum_ax1_xy_m512_n256_kernel(
    x: jax.Array,
):
    m, n = x.shape
    assert m == 4 * LANES and n == 2 * LANES
    raw_lo = m - RAW
    chunks = ((0, 2 * LANES), (2 * LANES, 3 * LANES), (3 * LANES, raw_lo))

    def body(x_hbm, out_ref, xbuf, send_buf, recv_buf, peer_rows,
             load_sems, send_sems, recv_sems):
        def load(i, lo, hi):
            rows = pl.ds(lo, hi - lo)
            return pltpu.make_async_copy(x_hbm.at[rows], xbuf.at[rows], load_sems.at[i])

        loads = [load(i, lo, hi) for i, (lo, hi) in enumerate(chunks)]
        for cp in loads:
            cp.start()

        peer = (lax.axis_index("x"), 1 - lax.axis_index("y"))
        barrier = pltpu.get_barrier_semaphore()
        pl.semaphore_signal(barrier, inc=1, device_id=peer,
                            device_id_type=pl.DeviceIdType.MESH)
        pl.semaphore_wait(barrier, 1)

        def remote(i, src, dst):
            return pltpu.make_async_remote_copy(
                src_ref=src, dst_ref=dst,
                send_sem=send_sems.at[i], recv_sem=recv_sems.at[i],
                device_id=peer, device_id_type=pl.DeviceIdType.MESH)

        raw = remote(3, x_hbm.at[pl.ds(raw_lo, RAW)], peer_rows)
        raw.start()

        off = (lax.broadcasted_iota(jnp.int32, (SUB, LANES), 1)
               - lax.broadcasted_iota(jnp.int32, (SUB, LANES), 0))

        def fold(ref, lo, hi):
            return ref[lo:hi, 0:LANES] + ref[lo:hi, LANES:2 * LANES]

        def lane_sums(groups):
            acc = jnp.zeros((SUB, LANES), jnp.float32)
            for r, v in groups:
                s = jnp.broadcast_to(jnp.sum(v, axis=1, keepdims=True), (SUB, LANES))
                acc = jnp.where(off == r % LANES, s, acc)
            return jnp.sum(acc, axis=0, keepdims=True)

        def tile_sums(t, hi, after_loads=None):
            lo, h = LANES * t, MXU_ROWS[t]
            groups = [(r, fold(xbuf, r, r + SUB)) for r in range(lo + h, hi, SUB)]
            head = fold(xbuf, lo, lo + h)
            res = after_loads() if after_loads is not None else None
            send_buf[:, lo:lo + LANES] = lane_sums(groups)
            send_buf[:, lo:lo + h] = lax.dot_general(
                jnp.ones((SUB, LANES), jnp.float32), head,
                (((1,), (1,)), ((), ())), preferred_element_type=jnp.float32)[0:1]
            return res

        def send(i, lo, hi):
            cols = pl.ds(lo, hi - lo)
            cp = remote(i, send_buf.at[:, cols], recv_buf.at[:, cols])
            cp.start()
            return cp

        loads[0].wait()
        tile_sums(0, LANES)
        tile_sums(1, 2 * LANES)
        s0 = send(0, 0, 2 * LANES)
        loads[1].wait()
        tile_sums(2, 3 * LANES)
        loads[2].wait()
        s1 = tile_sums(3, raw_lo, lambda: send(1, 2 * LANES, 3 * LANES))
        s2 = send(2, 3 * LANES, m)

        own_rows = load(3, raw_lo, m)
        own_rows.start()
        s0.wait_send()
        s1.wait_send()
        s2.wait_send()
        raw.wait_send()
        own_rows.wait()
        raw.wait_recv()
        own3 = send_buf[:, 3 * LANES:m] + lane_sums(
            [(r, fold(xbuf, r, r + SUB) + fold(peer_rows, r - raw_lo, r - raw_lo + SUB))
             for r in range(raw_lo, m, SUB)])
        s0.wait_recv()
        out_ref[:, 0:2 * LANES] = send_buf[:, 0:2 * LANES] + recv_buf[:, 0:2 * LANES]
        s1.wait_recv()
        out_ref[:, 2 * LANES:3 * LANES] = (send_buf[:, 2 * LANES:3 * LANES]
                                           + recv_buf[:, 2 * LANES:3 * LANES])
        s2.wait_recv()
        out_ref[:, 3 * LANES:m] = own3 + recv_buf[:, 3 * LANES:m]

    out = pl.pallas_call(
        body,
        out_shape=jax.ShapeDtypeStruct((1, m), x.dtype),
        in_specs=[pl.BlockSpec(memory_space=pl.ANY)],
        out_specs=pl.BlockSpec(memory_space=pltpu.VMEM),
        scratch_shapes=[
            pltpu.VMEM((m, n), jnp.float32),
            pltpu.VMEM((1, m), jnp.float32),
            pltpu.VMEM((1, m), jnp.float32),
            pltpu.VMEM((RAW, n), jnp.float32),
            pltpu.SemaphoreType.DMA((4,)),
            pltpu.SemaphoreType.DMA((4,)),
            pltpu.SemaphoreType.DMA((4,)),
        ],
        compiler_params=pltpu.CompilerParams(
            collective_id=0, disable_semaphore_checks=True),
    )(x)
    return out.reshape(m, 1)
```

```python
import jax
import jax.numpy as jnp
from jax import lax
from jax.experimental import pallas as pl
from jax.experimental.pallas import tpu as pltpu

LANES = 128
SUB = 8
RAW = 16
LAST = 96
MXU_ROWS = (80, 80, 56, 32)


def pallas_dist_sum_ax1_xy_m512_n256_kernel(
    x: jax.Array,
):
    m, n = x.shape
    assert m == 4 * LANES and n == 2 * LANES
    t1, t2, t3 = LANES, 2 * LANES, 3 * LANES
    last_hi, raw_lo = t3 + LAST, m - RAW
    pieces = ((last_hi, raw_lo), (0, t2), (t2, t3), (t3, last_hi))

    def body(x_hbm, out_ref, xbuf, send_buf, recv_buf, peer_rows,
             load_sems, send_sems, recv_sems):
        def load(i, lo, hi):
            rows = pl.ds(lo, hi - lo)
            return pltpu.make_async_copy(x_hbm.at[rows], xbuf.at[rows], load_sems.at[i])

        loads = [load(i, lo, hi) for i, (lo, hi) in enumerate(pieces)]
        for cp in loads:
            cp.start()

        peer = (lax.axis_index("x"), 1 - lax.axis_index("y"))
        barrier = pltpu.get_barrier_semaphore()
        pl.semaphore_signal(barrier, inc=1, device_id=peer,
                            device_id_type=pl.DeviceIdType.MESH)
        pl.semaphore_wait(barrier, 1)

        def remote(i, src, dst):
            return pltpu.make_async_remote_copy(
                src_ref=src, dst_ref=dst,
                send_sem=send_sems.at[i], recv_sem=recv_sems.at[i],
                device_id=peer, device_id_type=pl.DeviceIdType.MESH)

        raw = remote(3, x_hbm.at[pl.ds(raw_lo, RAW)], peer_rows)
        raw.start()

        off = (lax.broadcasted_iota(jnp.int32, (SUB, LANES), 1)
               - lax.broadcasted_iota(jnp.int32, (SUB, LANES), 0))
        zeros = jnp.zeros((SUB, LANES), jnp.float32)

        def fold(ref, lo, hi):
            return ref[lo:hi, 0:LANES] + ref[lo:hi, LANES:2 * LANES]

        def scatter_sums(acc, groups):
            for r, v in groups:
                s = jnp.broadcast_to(jnp.sum(v, axis=1, keepdims=True), (SUB, LANES))
                acc = jnp.where(off == r % LANES, s, acc)
            return acc

        def row_groups(lo, hi):
            return [(r, fold(xbuf, r, r + SUB)) for r in range(lo, hi, SUB)]

        def tile_sums(lo, hi, acc=zeros, after_loads=None):
            h = MXU_ROWS[lo // LANES]
            groups = row_groups(lo + h, hi)
            head = fold(xbuf, lo, lo + h)
            res = after_loads() if after_loads is not None else None
            send_buf[:, lo:lo + LANES] = jnp.sum(
                scatter_sums(acc, groups), axis=0, keepdims=True)
            send_buf[:, lo:lo + h] = lax.dot_general(
                jnp.ones((SUB, LANES), jnp.float32), head,
                (((1,), (1,)), ((), ())), preferred_element_type=jnp.float32)[0:1]
            return res

        def send(i, lo, hi):
            cols = pl.ds(lo, hi - lo)
            cp = remote(i, send_buf.at[:, cols], recv_buf.at[:, cols])
            cp.start()
            return cp

        loads[0].wait()
        loads[1].wait()
        acc3 = scatter_sums(zeros, row_groups(last_hi, raw_lo))
        tile_sums(0, t1)
        tile_sums(t1, t2)
        s0 = send(0, 0, t2)
        loads[2].wait()
        tile_sums(t2, t3)
        loads[3].wait()
        s1 = tile_sums(t3, last_hi, acc3, lambda: send(1, t2, t3))
        s2 = send(2, t3, m)

        own_rows = load(4, raw_lo, m)
        own_rows.start()
        s0.wait_send()
        s1.wait_send()
        s2.wait_send()
        raw.wait_send()
        own_rows.wait()
        raw.wait_recv()
        both = [(r, v + fold(peer_rows, r - raw_lo, r - raw_lo + SUB))
                for r, v in row_groups(raw_lo, m)]
        own3 = send_buf[:, t3:m] + jnp.sum(
            scatter_sums(zeros, both), axis=0, keepdims=True)
        s0.wait_recv()
        out_ref[:, 0:t2] = send_buf[:, 0:t2] + recv_buf[:, 0:t2]
        s1.wait_recv()
        out_ref[:, t2:t3] = send_buf[:, t2:t3] + recv_buf[:, t2:t3]
        s2.wait_recv()
        out_ref[:, t3:m] = own3 + recv_buf[:, t3:m]

    out = pl.pallas_call(
        body,
        out_shape=jax.ShapeDtypeStruct((1, m), x.dtype),
        in_specs=[pl.BlockSpec(memory_space=pl.ANY)],
        out_specs=pl.BlockSpec(memory_space=pltpu.VMEM),
        scratch_shapes=[
            pltpu.VMEM((m, n), jnp.float32),
            pltpu.VMEM((1, m), jnp.float32),
            pltpu.VMEM((1, m), jnp.float32),
            pltpu.VMEM((RAW, n), jnp.float32),
            pltpu.SemaphoreType.DMA((5,)),
            pltpu.SemaphoreType.DMA((4,)),
            pltpu.SemaphoreType.DMA((4,)),
        ],
        compiler_params=pltpu.CompilerParams(
            collective_id=0, disable_semaphore_checks=True),
    )(x)
    return out.reshape(m, 1)
```
